```python
import numpy as np

kernel_name = "dist_moe_cap_ep_tokshard_n2048_d512_e8_h1024"

def setup_inputs():
    x = np.random.randn(8192, 512).astype(np.float32)
    router_W = np.random.randn(512, 32).astype(np.float32) * 0.1
    scores64 = x.astype(np.float64) @ router_W.astype(np.float64)
    route_idx = np.argsort(-scores64, axis=-1)[:, :1].astype(np.int32)
    expert_W = np.random.randn(32, 512, 1024).astype(np.float32) * 0.02
    return {"x": x, "router_W": router_W, "route_idx": route_idx, "expert_W": expert_W}

def reference(x, router_W, route_idx, expert_W):
    counts = np.zeros(32, dtype=np.int64)
    out = np.zeros((8192, 1024), dtype=np.float32)
    for i in range(8192):
        e = int(route_idx[i, 0])
        if counts[e] < 204:
            out[i] = x[i] @ expert_W[e]
            counts[e] += 1
    return out
```

```python
import jax
import jax.numpy as jnp
from jax import lax
from jax.experimental import pallas as pl
from jax.experimental.pallas import tpu as pltpu

N_DEV = 4
N_EXP = 32
E_LOC = N_EXP // N_DEV
CAP = 204
SEG = 208
TOK = 2048
D_IN = 512
D_OUT = 1024
LANES = 128
XR = D_IN // (2 * LANES)
YR = D_OUT // (2 * LANES)
N_ROWS = TOK // LANES

X_CHUNK = 256
BOUNDS = (4, 8, 12, 16)
NB = len(BOUNDS)
PRE_ROW = 7
N_EARLY = 4
N_LATE = E_LOC - N_EARLY
LOOKAHEAD = 2


def _mask(rightwards):
    m = 0
    for chip, experts in enumerate(rightwards):
        for e in experts:
            m |= 1 << (chip * E_LOC + e)
    return m - (1 << 32) if m >= (1 << 31) else m


DIR_X = _mask([(1, 4, 6), (0, 2, 4, 6), (0, 2, 3, 5, 7), (1, 3, 5, 7)])
DIR_Y_EARLY = _mask([(1,), (0, 2), (0, 2, 3), (1, 3)])
DIR_Y_LATE = tuple(
    _mask([(4, 6), (4, 6), (5, 7), (5, 7)]) for _ in range(NB)
)


def _pack(lo, hi):
    lo = pltpu.bitcast(lo.astype(jnp.bfloat16).astype(jnp.float32), jnp.uint32)
    hi = pltpu.bitcast(hi.astype(jnp.bfloat16).astype(jnp.float32), jnp.uint32)
    return (lo >> 16) | (hi & jnp.uint32(0xFFFF0000))


def _unpack(w):
    lo = pltpu.bitcast(w << 16, jnp.float32)
    hi = pltpu.bitcast(w & jnp.uint32(0xFFFF0000), jnp.float32)
    return lo, hi


def _body(
    x_hbm, route_hbm, w_hbm, out_hbm,
    route_v, pos_v, pos2_v, tiles_v, tab_v, xf, xp, sb, rlx, land, wf,
    yb, rly, rb, yt, of,
    pos_s, pos2_s, tab_s,
    misc_sem, x_sem, w_sem, out_sem, tile_sem, send_sem,
    x_recv, rlx_recv, ye_recv, rlye_recv, yl_recv, rlyl_recv,
):
    me = lax.axis_index("i")
    right = (me + 1) % N_DEV
    diag = (me + 2) % N_DEV
    left = (me + 3) % N_DEV

    def remote(src, dst, recv, dev):
        return pltpu.make_async_remote_copy(
            src, dst, send_sem, recv,
            device_id=(dev,), device_id_type=pl.DeviceIdType.MESH)

    route_cp = pltpu.make_async_copy(route_hbm, route_v, misc_sem.at[0])
    route_cp.start()
    barrier = pltpu.get_barrier_semaphore()
    for dev in (right, diag, left):
        pl.semaphore_signal(
            barrier, 1, device_id=(dev,), device_id_type=pl.DeviceIdType.MESH)

    def x_copy(c):
        rows = pl.ds(pl.multiple_of(c * X_CHUNK, X_CHUNK), X_CHUNK)
        return pltpu.make_async_copy(x_hbm.at[rows], xf.at[rows], x_sem.at[c])

    def w_copy(e):
        return pltpu.make_async_copy(w_hbm.at[e], wf.at[e], w_sem.at[e])

    for c in range(TOK // X_CHUNK):
        x_copy(c).start()
    rb[pl.ds(N_EXP * SEG * YR, 8), :] = jnp.zeros((8, LANES), jnp.uint32)
    route_cp.wait()

    route = route_v[...] & (N_EXP - 1)
    exp_id = lax.broadcasted_iota(jnp.int32, (N_EXP, LANES), 0)
    lane = lax.broadcasted_iota(jnp.int32, (N_EXP, LANES), 1)
    onehot = [
        jnp.where(route[c:c + 1, :] == exp_id, 1.0, 0.0) for c in range(N_ROWS)
    ]
    k_id = lax.broadcasted_iota(jnp.int32, (LANES, 2 * LANES), 0)
    n_id = lax.broadcasted_iota(jnp.int32, (LANES, 2 * LANES), 1)
    tri = jnp.where(k_id < n_id, 1.0, 0.0).astype(jnp.bfloat16)
    sums = jnp.dot(
        jnp.concatenate(onehot, axis=0).astype(jnp.bfloat16), tri,
        preferred_element_type=jnp.float32)
    base = jnp.zeros((N_EXP, LANES), jnp.float32)
    counts = jnp.zeros((N_EXP, LANES), jnp.float32)
    ranks = []
    for c in range(N_ROWS):
        s = sums[c * N_EXP:(c + 1) * N_EXP]
        ranks.append(jnp.sum(
            onehot[c] * (s[:, :LANES] + base), axis=0, keepdims=True))
        base = base + s[:, LANES:]
        if c + 1 in BOUNDS:
            counts = jnp.where(lane == BOUNDS.index(c + 1), base, counts)
    rank = jnp.concatenate(ranks, axis=0).astype(jnp.int32)
    slot = route * SEG + jnp.minimum(rank, SEG - 1)
    pos_v[...] = slot * XR
    pos_cp = pltpu.make_async_copy(pos_v, pos_s, misc_sem.at[1])
    pos_cp.start()
    tile = jnp.concatenate([counts] * N_DEV, axis=0).T[:8]
    tiles_v[me] = tile.astype(jnp.int32)

    def tile_copy(k, src_dev, dev):
        return remote(
            tiles_v.at[src_dev], tiles_v.at[src_dev], tile_sem.at[k], dev)

    pl.semaphore_wait(barrier, N_DEV - 1)
    for k, dev in enumerate((right, diag, left)):
        tile_copy(k, me, dev).start()

    def scatter_chunk(c, carry):
        x_copy(c).wait()
        for g in range(X_CHUNK // 8):
            r = pl.multiple_of(c * X_CHUNK + g * 8, 8)
            v = xf[pl.ds(r, 8), :]
            for h in range(XR):
                xp[pl.ds(r * XR + h, 8, stride=XR), :] = _pack(
                    v[:, 2 * h * LANES:(2 * h + 1) * LANES],
                    v[:, (2 * h + 1) * LANES:(2 * h + 2) * LANES])

        def scatter(i, carry):
            row = c * (X_CHUNK // LANES) + i // 2
            col = (i % 2) * 64
            for u in range(64):
                t = row * LANES + col + u
                sb[pl.ds(pos_s[row, col + u], XR), :] = xp[pl.ds(t * XR, XR), :]
            return carry

        return lax.fori_loop(0, X_CHUNK // 64, scatter, carry)

    pos_cp.wait()
    lax.fori_loop(0, TOK // X_CHUNK, scatter_chunk, 0)
    for e in range(E_LOC):
        w_copy(e).start()

    for k, dev in enumerate((left, diag, right)):
        tile_copy(k, dev, dev).wait_recv()
    chip = lax.broadcasted_iota(jnp.int32, (8, LANES), 1) // N_EXP
    row = lax.broadcasted_iota(jnp.int32, (8, LANES), 0)
    cum = jnp.zeros((8, LANES), jnp.int32)
    pre = jnp.zeros((8, LANES), jnp.int32)
    for s in range(N_DEV):
        t = tiles_v[s]
        cum = jnp.where(chip == s, t, cum)
        pre = pre + jnp.where(chip > s, t[NB - 1:NB, :], 0)
    pre = jnp.minimum(pre, CAP)
    tab_v[...] = jnp.where(row == PRE_ROW, pre, jnp.minimum(cum, CAP - pre))
    tab_cp = pltpu.make_async_copy(tab_v, tab_s, misc_sem.at[2])
    tab_cp.start()
    tab_cp.wait()

    def span(s, g, j0, j1):
        col = s * N_EXP + g
        if isinstance(j0, int):
            lo = tab_s[j0 - 1, col] if j0 else 0
        else:
            lo = jnp.where(j0 > 0, tab_s[jnp.maximum(j0 - 1, 0), col], 0)
        return lo, tab_s[j1, col] - lo, tab_s[PRE_ROW, col]

    def rightwards(mask, s, e):
        return (lax.shift_right_logical(jnp.int32(mask), s * E_LOC + e) & 1) == 1

    def rows(ref, per, start, n):
        return ref.at[pl.ds(start * per, n * per)]

    def if_any(n, fn, cond=True):
        pl.when(jnp.logical_and(n > 0, cond))(fn)

    START, SENT, LANDED = range(3)

    def act_on(cp, act):
        if act == START:
            cp.start()
        elif act == SENT:
            cp.wait_send()
        else:
            cp.wait_recv()

    def x_last_hop(act, s, d, e, k, relay=None, cond=True):
        g = d * E_LOC + e
        lo, n, pre = span(s, g, 0, NB - 1)

        def go():
            if relay is None:
                src = rows(sb, XR, g * SEG + lo, n)
            else:
                src = rows(rlx, XR, (relay * E_LOC + e) * SEG + lo, n)
            dst = rows(land, XR, e * SEG + pre + lo, n)
            act_on(remote(src, dst, x_recv.at[k * E_LOC + e], d), act)

        if_any(n, go, cond)

    def x_first_hop(act, s, e, relay, cond=True):
        g = ((s + 2) % N_DEV) * E_LOC + e
        lo, n, _ = span(s, g, 0, NB - 1)

        def go():
            src = rows(sb, XR, g * SEG + lo, n)
            dst = rows(rlx, XR, (relay * E_LOC + e) * SEG + lo, n)
            via = (s + 1 + 2 * relay) % N_DEV
            act_on(remote(src, dst, rlx_recv.at[relay * E_LOC + e], via), act)

        if_any(n, go, cond)

    def x_local(act, e):
        g = me * E_LOC + e
        lo, n, pre = span(me, g, 0, NB - 1)

        def go():
            cp = pltpu.make_async_copy(
                rows(sb, XR, g * SEG + lo, n),
                rows(land, XR, e * SEG + pre + lo, n),
                x_recv.at[3 * E_LOC + e])
            cp.start() if act == START else cp.wait()

        if_any(n, go)

    def x_to_diag(act, e):
        x_first_hop(act, me, e, jnp.where(rightwards(DIR_X, me, e), 0, 1))

    def x_direct(act, e):
        x_last_hop(act, me, right, e, 0)
        x_last_hop(act, me, left, e, 1)

    def x_forward(act, e):
        for relay, (s, d) in enumerate(((left, right), (right, left))):
            cond = rightwards(DIR_X, s, e) == (relay == 0)
            if act == START:
                x_first_hop(LANDED, s, e, relay, cond)
            x_last_hop(act, s, d, e, 2, relay, cond)

    def x_landed(e):
        x_last_hop(LANDED, left, me, e, 0)
        x_last_hop(LANDED, right, me, e, 1)
        x_last_hop(LANDED, diag, me, e, 2)
        x_local(LANDED, e)

    def y_last_hop(act, s, d, e, j0, j1, sems, unit, k, relay=None, cond=True):
        g = d * E_LOC + e
        lo, n, pre = span(s, g, j0, j1)

        def go():
            if relay is None:
                src = rows(yb, YR, e * SEG + pre + lo, n)
            else:
                src = rows(rly, YR, (relay * E_LOC + e) * SEG + lo, n)
            dst = rows(rb, YR, g * SEG + lo, n)
            act_on(remote(src, dst, sems.at[unit * 4 + k], s), act)

        if_any(n, go, cond)

    def y_first_hop(act, d, e, j0, j1, sems, unit, relay, cond=True):
        lo, n, pre = span((d + 2) % N_DEV, d * E_LOC + e, j0, j1)

        def go():
            src = rows(yb, YR, e * SEG + pre + lo, n)
            dst = rows(rly, YR, (relay * E_LOC + e) * SEG + lo, n)
            via = (d + 1 + 2 * relay) % N_DEV
            act_on(remote(src, dst, sems.at[unit * 2 + relay], via), act)

        if_any(n, go, cond)

    def y_local(act, e, j0, j1, sems, unit):
        g = me * E_LOC + e
        lo, n, pre = span(me, g, j0, j1)

        def go():
            cp = pltpu.make_async_copy(
                rows(yb, YR, e * SEG + pre + lo, n),
                rows(rb, YR, g * SEG + lo, n),
                sems.at[unit * 4 + 3])
            cp.start() if act == START else cp.wait()

        if_any(n, go)

    class Combine:
        def __init__(self, e, j0, j1, mask, sems, relay_sems, unit):
            self.e, self.mask, self.relay_sems = e, mask, relay_sems
            self.at = (e, j0, j1)
            self.sem = (sems, unit)

        def to_diag(self, act):
            relay = jnp.where(rightwards(self.mask, me, self.e), 0, 1)
            y_first_hop(act, me, *self.at, self.relay_sems, self.sem[1], relay)

        def direct(self, act):
            y_last_hop(act, left, me, *self.at, *self.sem, 0)
            y_last_hop(act, right, me, *self.at, *self.sem, 1)

        def local(self):
            y_local(START, *self.at, *self.sem)

        def forward(self, act):
            for relay, (d, s) in enumerate(((left, right), (right, left))):
                cond = rightwards(self.mask, d, self.e) == (relay == 0)
                if act == START:
                    y_first_hop(LANDED, d, *self.at, self.relay_sems,
                                self.sem[1], relay, cond)
                y_last_hop(act, s, d, *self.at, *self.sem, 2, relay, cond)

        def landed(self):
            y_last_hop(LANDED, me, right, *self.at, *self.sem, 0)
            y_last_hop(LANDED, me, left, *self.at, *self.sem, 1)
            y_last_hop(LANDED, me, diag, *self.at, *self.sem, 2)
            y_local(LANDED, *self.at, *self.sem)

    def early(e):
        return Combine(e, 0, NB - 1, DIR_Y_EARLY, ye_recv, rlye_recv, e)

    def late(e, j):
        return Combine(e, j, j, DIR_Y_LATE[j], yl_recv, rlyl_recv,
                       j * N_LATE + e - N_EARLY)

    def loop(lo, hi, fn):
        lax.fori_loop(lo, hi, lambda i, c: (fn(i), c)[1], 0)

    loop(0, E_LOC, lambda e: x_to_diag(START, e))
    loop(0, LOOKAHEAD, lambda e: x_direct(START, e))
    loop(0, E_LOC, lambda e: x_local(START, e))

    def dispatch_step(e):
        x_forward(START, e)
        pl.when(e + LOOKAHEAD < E_LOC)(
            lambda: x_direct(START, jnp.minimum(e + LOOKAHEAD, E_LOC - 1)))

    loop(0, E_LOC, dispatch_step)

    pre_t = jnp.broadcast_to(pre[:1].astype(jnp.float32), (LANES, LANES)).T
    pre_me = jnp.zeros((N_EXP, LANES), jnp.float32)
    for s in range(N_DEV):
        pre_me = jnp.where(me == s, pre_t[s * N_EXP:(s + 1) * N_EXP], pre_me)
    before = jnp.concatenate(
        [jnp.sum(o * pre_me, axis=0, keepdims=True) for o in onehot], axis=0)
    kept = rank + before.astype(jnp.int32) < CAP
    pos2_v[...] = jnp.where(kept, slot, N_EXP * SEG) * YR
    pos2_cp = pltpu.make_async_copy(pos2_v, pos2_s, misc_sem.at[3])
    pos2_cp.start()

    def expert(e):
        w_copy(e).wait()
        x_landed(e)
        parts = []
        for h in range(XR):
            w = land[pl.ds(e * (SEG * XR) + h, SEG, stride=XR), :]
            parts += [p.astype(jnp.bfloat16) for p in _unpack(w)]
        y = jnp.dot(
            jnp.concatenate(parts, axis=1), wf[e].astype(jnp.bfloat16),
            preferred_element_type=jnp.float32)
        for h in range(YR):
            yb[pl.ds(e * (SEG * YR) + h, SEG, stride=YR), :] = _pack(
                y[:, 2 * h * LANES:(2 * h + 1) * LANES],
                y[:, (2 * h + 1) * LANES:(2 * h + 2) * LANES])

        @pl.when(e < N_EARLY)
        def _():
            unit = early(jnp.minimum(e, N_EARLY - 1))
            unit.to_diag(START)
            unit.direct(START)
            unit.local()

    loop(0, E_LOC, expert)

    def out_copy(j):
        lo = (BOUNDS[j - 1] if j else 0) * LANES
        blk = pl.ds(lo, BOUNDS[j] * LANES - lo)
        return pltpu.make_async_copy(of.at[blk], out_hbm.at[blk], out_sem.at[j])

    def finish_block(j):
        if j == 0:
            loop(0, N_EARLY, lambda e: early(e).landed())
            pos2_cp.wait()
        loop(N_EARLY, E_LOC, lambda e: late(e, j).landed())

        def gather(i):
            row = i // 2
            col = (i % 2) * 64
            t0 = pl.multiple_of(i * 64, 64)
            for u in range(64):
                yt[pl.ds((t0 + u) * YR, YR), :] = rb[
                    pl.ds(pos2_s[row, col + u], YR), :]
            for g in range(8):
                r = pl.multiple_of(t0 + g * 8, 8)
                for h in range(YR):
                    lo, hi = _unpack(yt[pl.ds(r * YR + h, 8, stride=YR), :])
                    of[pl.ds(r, 8), 2 * h * LANES:(2 * h + 1) * LANES] = lo
                    of[pl.ds(r, 8), (2 * h + 1) * LANES:(2 * h + 2) * LANES] = hi

        loop(2 * (BOUNDS[j - 1] if j else 0), 2 * BOUNDS[j], gather)
        out_copy(j).start()

    loop(N_EARLY, E_LOC, lambda e: late(e, 0).to_diag(START))
    loop(0, N_EARLY, lambda e: early(e).forward(START))
    for j in range(NB):
        if j + 1 < NB:
            loop(N_EARLY, E_LOC, lambda e: late(e, j + 1).to_diag(START))

        def direct(e):
            unit = late(e, j)
            unit.direct(START)
            unit.local()

        loop(N_EARLY, E_LOC, direct)
        loop(N_EARLY, E_LOC, lambda e: late(e, j).forward(START))
        if j:
            finish_block(j - 1)
    finish_block(NB - 1)

    for k, dev in enumerate((right, diag, left)):
        tile_copy(k, me, dev).wait_send()

    def x_sent(e):
        x_to_diag(SENT, e)
        x_direct(SENT, e)
        x_forward(SENT, e)

    def y_sent(unit):
        unit.to_diag(SENT)
        unit.direct(SENT)
        unit.forward(SENT)

    loop(0, E_LOC, x_sent)
    loop(0, N_EARLY, lambda e: y_sent(early(e)))
    for j in range(NB):
        loop(N_EARLY, E_LOC, lambda e: y_sent(late(e, j)))
        out_copy(j).wait()


def pallas_dist_moe_cap_ep_tokshard_n2048_d512_e8_h1024_kernel(
    x: jax.Array,
    router_W: jax.Array,
    route_idx: jax.Array,
    expert_W: jax.Array,
):
    del router_W
    route = route_idx.astype(jnp.int32).reshape(N_ROWS, LANES)
    dma = pltpu.SemaphoreType.DMA
    i32, u32, f32 = jnp.int32, jnp.uint32, jnp.float32
    hbm = pl.BlockSpec(memory_space=pltpu.HBM)
    return pl.pallas_call(
        _body,
        out_shape=jax.ShapeDtypeStruct((TOK, D_OUT), f32),
        in_specs=[hbm, hbm, hbm],
        out_specs=hbm,
        scratch_shapes=[
            pltpu.VMEM((N_ROWS, LANES), i32),
            pltpu.VMEM((N_ROWS, LANES), i32),
            pltpu.VMEM((N_ROWS, LANES), i32),
            pltpu.VMEM((N_DEV, 8, LANES), i32),
            pltpu.VMEM((8, LANES), i32),
            pltpu.VMEM((TOK, D_IN), f32),
            pltpu.VMEM((TOK * XR, LANES), u32),
            pltpu.VMEM((N_EXP * SEG * XR, LANES), u32),
            pltpu.VMEM((2 * E_LOC * SEG * XR, LANES), u32),
            pltpu.VMEM((E_LOC * SEG * XR, LANES), u32),
            pltpu.VMEM((E_LOC, D_IN, D_OUT), f32),
            pltpu.VMEM((E_LOC * SEG * YR, LANES), u32),
            pltpu.VMEM((2 * E_LOC * SEG * YR, LANES), u32),
            pltpu.VMEM((N_EXP * SEG * YR + 8, LANES), u32),
            pltpu.VMEM((TOK * YR, LANES), u32),
            pltpu.VMEM((TOK, D_OUT), f32),
            pltpu.SMEM((N_ROWS, LANES), i32),
            pltpu.SMEM((N_ROWS, LANES), i32),
            pltpu.SMEM((8, LANES), i32),
            dma((4,)),
            dma((TOK // X_CHUNK,)),
            dma((E_LOC,)),
            dma((NB,)),
            dma((N_DEV - 1,)),
            dma,
            dma((4 * E_LOC,)),
            dma((2 * E_LOC,)),
            dma((4 * N_EARLY,)),
            dma((2 * N_EARLY,)),
            dma((4 * N_LATE * NB,)),
            dma((2 * N_LATE * NB,)),
        ],
        compiler_params=pltpu.CompilerParams(
            collective_id=0, vmem_limit_bytes=100 * 1024 * 1024),
    )(x, route, expert_W)
```

```python
import jax
import jax.numpy as jnp
from jax import lax
from jax.experimental import pallas as pl
from jax.experimental.pallas import tpu as pltpu

N_DEV = 4
N_EXP = 32
E_LOC = N_EXP // N_DEV
CAP = 204
SEG = 208
TOK = 2048
D_IN = 512
D_OUT = 1024
LANES = 128
XR = D_IN // (2 * LANES)
YR = D_OUT // (2 * LANES)
OR = D_OUT // LANES
N_ROWS = TOK // LANES

X_CHUNK = 256
HEAD_CHUNKS = 2
ALL_ROW, HEAD_ROW, PRE_ROW, RAW_ROW = 0, 1, 2, 3
RAW_HEAD_ROW = RAW_ROW + HEAD_CHUNKS - 1
HEAD, TAIL, WHOLE = range(3)
LOOKAHEAD = 1
BATCH = 8

X_RIGHT = [(0, 2, 4, 6, 7), (0, 2, 4, 6, 7), (2, 4, 6), (0, 2, 3, 4, 5, 6, 7)]
X_MASK = sum(1 << (c * E_LOC + e) for c in range(N_DEV) for e in X_RIGHT[c])
X_MASK -= (X_MASK >> 31) << 32
WARMUP = 560
BIAS_RIGHT = (10, -5, 0, 15)
BIAS_LEFT = (95, -30, -15, -25)


def _pack(lo, hi):
    lo = pltpu.bitcast(lo.astype(jnp.bfloat16).astype(jnp.float32), jnp.uint32)
    hi = pltpu.bitcast(hi.astype(jnp.bfloat16).astype(jnp.float32), jnp.uint32)
    return (lo >> 16) | (hi & jnp.uint32(0xFFFF0000))


def _unpack(w):
    lo = pltpu.bitcast(w << 16, jnp.float32)
    hi = pltpu.bitcast(w & jnp.uint32(0xFFFF0000), jnp.float32)
    return lo, hi


def _loop(lo, hi, fn):
    def step(i, carry):
        fn(i)
        return carry

    lax.fori_loop(lo, hi, step, 0)


def _rows(ref, per, first, n):
    return ref.at[pl.ds(first * per, n * per)]


def _wait_filled(ref, per, first, n, sem):
    @pl.when(n > 0)
    def _():
        buf = _rows(ref, per, first, n)
        pltpu.make_async_copy(buf, buf, sem).wait()


def _body(
    x_hbm, route_hbm, w_hbm, out,
    route_v, pos_v, tiles_v, tab_v, xf, xp, sb, rlx, land, wf,
    yb, rly, rb, rbd,
    pos_s, tab_s, row_s, share_s,
    last_sem, rbd_sem,
):
    me = lax.axis_index("i")
    right = (me + 1) % N_DEV
    diag = (me + 2) % N_DEV
    left = (me + 3) % N_DEV

    def remote(send_sem, src, dst, recv_sem, dev):
        return pltpu.make_async_remote_copy(
            src, dst, send_sem, recv_sem,
            device_id=(dev,), device_id_type=pl.DeviceIdType.MESH)

    START, SENT = range(2)

    def sender(send_sem):
        def send(act, per, n, src, src_at, dst, dst_at, recv_sem, dev):
            @pl.when(n > 0)
            def _():
                cp = remote(send_sem, _rows(src, per, src_at, n),
                            _rows(dst, per, dst_at, n), recv_sem, dev)
                cp.start() if act == START else cp.wait_send()

        return send

    def span(s, g, part=WHOLE):
        col = s * N_EXP + g
        lo = tab_s[HEAD_ROW, col] if part == TAIL else 0
        hi = tab_s[HEAD_ROW if part == HEAD else ALL_ROW, col]
        return lo, hi - lo, tab_s[PRE_ROW, col]

    def middle(e):
        return (2 * e + 1) * SEG

    def y_split(d, e):
        n = span((d + 2) % N_DEV, d * E_LOC + e)[1]
        return n, (n * share_s[d] + 128) >> 8

    def y_relayed(e):
        n1, k1 = y_split(right, e)
        return y_split(left, e)[1], k1, n1

    def y_forward(act, e):
        k0, k1, n1 = y_relayed(e)
        send = sender(last_sem)
        send(act, YR, k0, rly, middle(e) - k0, rbd, e * SEG, rbd_sem.at[e], right)
        send(act, YR, n1 - k1, rly, middle(e), rbd, e * SEG + k1, rbd_sem.at[e], left)

    def place(buf, first, g, n):
        def some(i, count):
            rs = [row_s[g * SEG + i + u] for u in range(count)]
            for u, r in enumerate(rs):
                lo, hi = _unpack(buf[pl.ds((first + i + u) * YR, YR), :])
                out[pl.ds(r, YR, stride=8), :] = lo
                out[pl.ds(r + 8 * YR, YR, stride=8), :] = hi

        _loop(0, n // BATCH, lambda i: some(i * BATCH, BATCH))
        _loop(n // BATCH * BATCH, n, lambda i: some(i, 1))

    def all_but_last_results(
        misc_sem, load_sem, send_sem, tile_sem, land_sem, rlx_sem, rly_sem, rb_sem
    ):
        send = sender(send_sem)

        route_cp = pltpu.make_async_copy(route_hbm, route_v, misc_sem)
        route_cp.start()
        barrier = pltpu.get_barrier_semaphore()
        for dev in (right, diag, left):
            pl.semaphore_signal(
                barrier, 1, device_id=(dev,), device_id_type=pl.DeviceIdType.MESH)

        def x_copy(c):
            chunk = pl.ds(pl.multiple_of(c * X_CHUNK, X_CHUNK), X_CHUNK)
            return pltpu.make_async_copy(x_hbm.at[chunk], xf.at[chunk], load_sem.at[c])

        def w_copy(e):
            return pltpu.make_async_copy(w_hbm.at[e], wf.at[e], load_sem.at[e])

        for c in range(TOK // X_CHUNK):
            x_copy(c).start()
        route_cp.wait()

        route = route_v[...] & (N_EXP - 1)
        exp_id = lax.broadcasted_iota(jnp.int32, (N_EXP, LANES), 0)
        onehot = [
            jnp.where(route[c:c + 1, :] == exp_id, 1.0, 0.0) for c in range(N_ROWS)
        ]
        k_id = lax.broadcasted_iota(jnp.int32, (LANES, 2 * LANES), 0)
        n_id = lax.broadcasted_iota(jnp.int32, (LANES, 2 * LANES), 1)
        tri = jnp.where(k_id < n_id, 1.0, 0.0).astype(jnp.bfloat16)
        sums = jnp.dot(
            jnp.concatenate(onehot, axis=0).astype(jnp.bfloat16), tri,
            preferred_element_type=jnp.float32)
        base = jnp.zeros((N_EXP, LANES), jnp.float32)
        ranks, so_far = [], []
        for c in range(N_ROWS):
            s = sums[c * N_EXP:(c + 1) * N_EXP]
            ranks.append(jnp.sum(
                onehot[c] * (s[:, :LANES] + base), axis=0, keepdims=True))
            base = base + s[:, LANES:]
            if (c + 1) * LANES % X_CHUNK == 0:
                so_far.append(base)
        rank = jnp.concatenate(ranks, axis=0).astype(jnp.int32)
        lane = lax.broadcasted_iota(jnp.int32, (N_EXP, LANES), 1)
        counts = jnp.where(lane == HEAD_ROW, so_far[HEAD_CHUNKS - 1], base)
        for c in range(HEAD_CHUNKS):
            counts = jnp.where(lane == RAW_ROW + c, so_far[c], counts)
        tile = jnp.concatenate([counts] * N_DEV, axis=0).T[:8].astype(jnp.int32)
        tiles_v[0] = tile
        pos_v[:N_ROWS] = (route * SEG + jnp.minimum(rank, SEG - 1)) * XR
        pos_v[N_ROWS:] = jnp.minimum(tile, CAP)
        pos_cp = pltpu.make_async_copy(pos_v, pos_s, misc_sem)
        pos_cp.start()

        def tile_copy(k):
            dev = (me + N_DEV - k) % N_DEV
            return remote(send_sem, tiles_v.at[0], tiles_v.at[k], tile_sem, dev)

        def scatter_chunk(c):
            x_copy(c).wait()

            @pl.when(c == TOK // X_CHUNK - 1)
            def _():
                for e in range(E_LOC):
                    w_copy(e).start()

            for g in range(X_CHUNK // 8):
                r = pl.multiple_of(c * X_CHUNK + g * 8, 8)
                v = xf[pl.ds(r, 8), :]
                for h in range(XR):
                    xp[pl.ds(r * XR + h, 8, stride=XR), :] = _pack(
                        v[:, 2 * h * LANES:(2 * h + 1) * LANES],
                        v[:, (2 * h + 1) * LANES:(2 * h + 2) * LANES])

            def scatter(i):
                row = c * (X_CHUNK // LANES) + i
                t0 = pl.multiple_of(row * (LANES * XR), LANES * XR)
                for u0 in range(0, LANES, BATCH):
                    ps = [pos_s[row, u0 + u] for u in range(BATCH)]
                    for u, p in enumerate(ps):
                        sb[pl.ds(p, XR), :] = xp[pl.ds(t0 + (u0 + u) * XR, XR), :]

            _loop(0, X_CHUNK // LANES, scatter)

        def x_side(chip, e):
            bit = lax.shift_right_logical(jnp.int32(X_MASK), chip * E_LOC + e)
            return 1 - (bit & 1)

        def x_to_diag(act, e, lo, hi):
            side = x_side(me, e)
            send(act, XR, hi - lo, sb, (diag * E_LOC + e) * SEG + lo,
                 rlx, (2 * e + side) * SEG + lo, rlx_sem.at[2 * e + side],
                 (me + 1 + 2 * side) % N_DEV)

        def x_chunk_to_diag(act, c, e):
            g = diag * E_LOC + e
            lo = pos_s[N_ROWS + RAW_ROW + c - 1, g] if c else 0
            x_to_diag(act, e, lo, pos_s[N_ROWS + RAW_ROW + c, g])

        pos_cp.wait()
        for c in range(HEAD_CHUNKS):
            _loop(c, c + 1, scatter_chunk)
            if c == 0:
                pl.semaphore_wait(barrier, N_DEV - 1)
                for k in (2, 1, 3):
                    tile_copy(k).start()
            _loop(0, E_LOC, lambda e: x_chunk_to_diag(START, c, e))

        def x_head_of_first_chip(e):
            for dev in (right, left):
                g = dev * E_LOC + e
                send(START, XR, pos_s[N_ROWS + RAW_HEAD_ROW, g],
                     sb, g * SEG, land, e * SEG, land_sem.at[e], dev)

        pl.when(me == 0)(lambda: _loop(0, E_LOC, x_head_of_first_chip))

        others = tiles_v.at[pl.ds(1, N_DEV - 1)]
        pltpu.make_async_copy(others, others, tile_sem).wait()
        chip = lax.broadcasted_iota(jnp.int32, (8, LANES), 1) // N_EXP
        row = lax.broadcasted_iota(jnp.int32, (8, LANES), 0)
        cum = jnp.zeros((8, LANES), jnp.int32)
        pre = jnp.zeros((8, LANES), jnp.int32)
        for k in range(N_DEV):
            s = (me + k) % N_DEV
            t = tiles_v[k]
            cum = jnp.where(chip == s, t, cum)
            pre = pre + jnp.where(chip > s, t[ALL_ROW:ALL_ROW + 1], 0)
        pre = jnp.minimum(pre, CAP)
        room = jnp.where(row >= RAW_ROW, CAP, CAP - pre)
        tab_v[...] = jnp.where(row == PRE_ROW, pre, jnp.minimum(cum, room))
        tab_cp = pltpu.make_async_copy(tab_v, tab_s, misc_sem)
        tab_cp.start()
        tab_cp.wait()

        def x_ends(s, d, e, part=WHOLE):
            g = d * E_LOC + e
            lo, n, pre = span(s, g, part)
            return n, sb, g * SEG + lo, land, e * SEG + pre + lo, land_sem.at[e]

        def x_tail_to_diag(act, e):
            col = me * N_EXP + diag * E_LOC + e
            x_to_diag(act, e, tab_s[RAW_HEAD_ROW, col], tab_s[ALL_ROW, col])

        def x_direct(act, e, part):
            for dev in (right, left):
                send(act, XR, *x_ends(me, dev, e, part), dev)

        def x_forward(act, e):
            for side, (frm, to) in enumerate(((left, right), (right, left))):
                n, _, _, *dst = x_ends(frm, to, e)
                here = x_side(frm, e) == side
                at = (2 * e + side) * SEG
                if act == START:
                    raw = tab_s[RAW_HEAD_ROW, frm * N_EXP + to * E_LOC + e]
                    _wait_filled(rlx, XR, at, jnp.where(here, jnp.maximum(n, raw), 0),
                                 rlx_sem.at[2 * e + side])
                send(act, XR, jnp.where(here, n, 0), rlx, at, *dst, to)

        def x_own(e):
            n, src, src_at, dst, dst_at, sem = x_ends(me, me, e)

            @pl.when(n > 0)
            def _():
                pltpu.make_async_copy(
                    _rows(src, XR, src_at, n), _rows(dst, XR, dst_at, n), sem).start()

        def y_to_diag(act, e):
            n, k = y_split(me, e)
            at = e * SEG + span(diag, me * E_LOC + e)[2]
            send(act, YR, k, yb, at, rly, middle(e) - k, rly_sem.at[e], right)
            send(act, YR, n - k, yb, at + k, rly, middle(e), rly_sem.at[e], left)

        def y_direct(act, e):
            _, n, pre = span(right, me * E_LOC + e)
            send(act, YR, n, yb, e * SEG + pre, rb, middle(e) - n, rb_sem.at[e], right)
            _, n, pre = span(left, me * E_LOC + e)
            send(act, YR, n, yb, e * SEG + pre, rb, middle(e), rb_sem.at[e], left)

        def balance():
            chips = range(N_DEV)
            w = YR // XR

            def kept(s, d, experts=range(E_LOC)):
                first = s % N_DEV * N_EXP + d % N_DEV * E_LOC
                return sum(tab_s[ALL_ROW, first + e] for e in experts)

            to_r = [kept(m, m + 1) for m in chips]
            to_l = [kept(m, m - 1) for m in chips]
            to_d = [kept(m, m + 2) for m in chips]
            via_r = [kept(m, m + 2, X_RIGHT[m]) for m in chips]
            via_l = [to_d[m] - via_r[m] for m in chips]
            link_r = [
                jnp.maximum(to_r[m] + via_r[m] + via_r[m - 1], WARMUP)
                + w * to_l[(m + 1) % N_DEV] + BIAS_RIGHT[m] for m in chips]
            link_l = [
                jnp.maximum(to_l[m] + via_l[m] + via_l[(m + 1) % N_DEV], WARMUP)
                + w * to_r[m - 1] + BIAS_LEFT[m] for m in chips]
            todo = [w * to_d[(m + 2) % N_DEV] for m in chips]
            cut = [link_r[m] + link_l[m - 1] + todo[m - 1] + todo[m] for m in chips]
            add = [(cut[m] >> 1) - link_r[m] for m in chips]
            gap = add[0] + add[2] - add[1] - add[3]
            worst = jnp.maximum(jnp.maximum(cut[0], cut[1]),
                                jnp.maximum(cut[2], cut[3]))
            slack = [(worst - cut[m]) >> 1 for m in chips]
            total = sum(slack)
            used = jnp.minimum(jnp.abs(gap), total)
            for m in chips:
                give = (lax.div(used * slack[m], jnp.maximum(total, 1))
                        + ((jnp.abs(gap) - used) >> 2))
                add[m] += jnp.where((gap > 0) == (m % 2 == 0), -give, give)
            c1, c2, c3 = add[1], add[2] - add[1], add[3] - add[2] + add[1]
            lo = jnp.maximum(jnp.maximum(c1 - todo[1], -c2),
                             jnp.maximum(c3 - todo[3], 0))
            hi = jnp.minimum(jnp.minimum(todo[0], c1),
                             jnp.minimum(todo[2] - c2, c3))
            t = (lo + hi) >> 1
            for m, a in enumerate((t, c1 - t, c2 + t, c3 - t)):
                share = lax.div(jnp.maximum(a, 0) * 256, jnp.maximum(todo[m], 1))
                share_s[m] = jnp.minimum(share, 256)

        pl.when(me > 0)(
            lambda: _loop(0, E_LOC, lambda e: x_direct(START, e, HEAD)))
        _loop(HEAD_CHUNKS, TOK // X_CHUNK, scatter_chunk)
        _loop(0, E_LOC, lambda e: x_tail_to_diag(START, e))
        _loop(0, LOOKAHEAD, lambda e: x_direct(START, e, TAIL))
        _loop(0, E_LOC, x_own)
        balance()

        def dispatch_step(e):
            x_forward(START, e)
            pl.when(e + LOOKAHEAD < E_LOC)(lambda: x_direct(
                START, jnp.minimum(e + LOOKAHEAD, E_LOC - 1), TAIL))

        _loop(0, E_LOC, dispatch_step)

        def expert(e):
            w_copy(e).wait()
            _, n_last, pre_last = span(N_DEV - 1, me * E_LOC + e)
            n = pre_last + n_last
            _wait_filled(land, XR, e * SEG, n, land_sem.at[e])
            filled = lax.broadcasted_iota(jnp.int32, (SEG, LANES), 0) < n
            parts = []
            for h in range(XR):
                w = land[pl.ds(e * (SEG * XR) + h, SEG, stride=XR), :]
                w = jnp.where(filled, w, jnp.uint32(0))
                parts += [p.astype(jnp.bfloat16) for p in _unpack(w)]
            y = jnp.dot(
                jnp.concatenate(parts, axis=1), wf[e].astype(jnp.bfloat16),
                preferred_element_type=jnp.float32)
            for h in range(YR):
                yb[pl.ds(e * (SEG * YR) + h, SEG, stride=YR), :] = _pack(
                    y[:, h * LANES:(h + 1) * LANES],
                    y[:, (YR + h) * LANES:(YR + h + 1) * LANES])
            y_to_diag(START, e)
            y_direct(START, e)

        _loop(0, E_LOC, expert)

        def clear(i):
            r = pl.multiple_of(i * 256, 256)
            out[pl.ds(r, 256), :] = jnp.zeros((256, LANES), jnp.float32)

        def invert(row):
            for u0 in range(0, LANES, BATCH):
                ps = [pos_s[row, u0 + u] for u in range(BATCH)]
                for u, p in enumerate(ps):
                    t = u0 + u
                    first = row * (LANES * OR) + (t // 8) * (8 * OR) + t % 8
                    row_s[lax.shift_right_logical(p, 1)] = first

        _loop(0, TOK * OR // 256, clear)
        _loop(0, N_ROWS, invert)

        def place_own(e):
            _, n, pre = span(me, me * E_LOC + e)
            place(yb, e * SEG + pre, me * E_LOC + e, n)

        _loop(0, E_LOC, place_own)
        for k in range(1, N_DEV):
            tile_copy(k).wait_send()

        def x_sent(e):
            for c in range(HEAD_CHUNKS):
                x_chunk_to_diag(SENT, c, e)
            x_tail_to_diag(SENT, e)
            x_direct(SENT, e, HEAD)
            x_direct(SENT, e, TAIL)
            x_forward(SENT, e)

        _loop(0, E_LOC, x_sent)

        def from_neighbours(e):
            k0, k1, n1 = y_relayed(e)
            _wait_filled(rly, YR, middle(e) - k0, k0 + n1 - k1, rly_sem.at[e])
            y_forward(START, e)
            g0, g1 = left * E_LOC + e, right * E_LOC + e
            n0, n1 = span(me, g0)[1], span(me, g1)[1]
            _wait_filled(rb, YR, middle(e) - n0, n0 + n1, rb_sem.at[e])
            place(rb, middle(e) - n0, g0, n0)
            place(rb, middle(e), g1, n1)

        def y_sent(e):
            y_to_diag(SENT, e)
            y_direct(SENT, e)

        _loop(0, E_LOC, from_neighbours)
        _loop(0, E_LOC, y_sent)

    dma = pltpu.SemaphoreType.DMA
    pl.run_scoped(
        all_but_last_results,
        misc_sem=dma,
        load_sem=dma((max(TOK // X_CHUNK, E_LOC),)),
        send_sem=dma,
        tile_sem=dma,
        land_sem=dma((E_LOC,)),
        rlx_sem=dma((2 * E_LOC,)),
        rly_sem=dma((E_LOC,)),
        rb_sem=dma((E_LOC,)),
    )

    def from_diag(e):
        y_forward(SENT, e)
        g = diag * E_LOC + e
        n = span(me, g)[1]
        _wait_filled(rbd, YR, e * SEG, n, rbd_sem.at[e])
        place(rbd, e * SEG, g, n)

    _loop(0, E_LOC, from_diag)


def pallas_dist_moe_cap_ep_tokshard_n2048_d512_e8_h1024_kernel(
    x: jax.Array,
    router_W: jax.Array,
    route_idx: jax.Array,
    expert_W: jax.Array,
):
    del router_W
    route = route_idx.astype(jnp.int32).reshape(N_ROWS, LANES)
    dma = pltpu.SemaphoreType.DMA
    i32, u32, f32 = jnp.int32, jnp.uint32, jnp.float32
    hbm = pl.BlockSpec(memory_space=pltpu.HBM)
    out = pl.pallas_call(
        _body,
        out_shape=jax.ShapeDtypeStruct((TOK * OR, LANES), f32),
        in_specs=[hbm, hbm, hbm],
        out_specs=pl.BlockSpec(memory_space=pltpu.VMEM),
        scratch_shapes=[
            pltpu.VMEM((N_ROWS, LANES), i32),
            pltpu.VMEM((N_ROWS + 8, LANES), i32),
            pltpu.VMEM((N_DEV, 8, LANES), i32),
            pltpu.VMEM((8, LANES), i32),
            pltpu.VMEM((TOK, D_IN), f32),
            pltpu.VMEM((TOK * XR, LANES), u32),
            pltpu.VMEM((N_EXP * SEG * XR, LANES), u32),
            pltpu.VMEM((2 * E_LOC * SEG * XR, LANES), u32),
            pltpu.VMEM((E_LOC * SEG * XR, LANES), u32),
            pltpu.VMEM((E_LOC, D_IN, D_OUT), f32),
            pltpu.VMEM((E_LOC * SEG * YR, LANES), u32),
            pltpu.VMEM((2 * E_LOC * SEG * YR, LANES), u32),
            pltpu.VMEM((2 * E_LOC * SEG * YR, LANES), u32),
            pltpu.VMEM((E_LOC * SEG * YR, LANES), u32),
            pltpu.SMEM((N_ROWS + 8, LANES), i32),
            pltpu.SMEM((8, LANES), i32),
            pltpu.SMEM((N_EXP * SEG,), i32),
            pltpu.SMEM((N_DEV,), i32),
            dma,
            dma((E_LOC,)),
        ],
        compiler_params=pltpu.CompilerParams(
            collective_id=0, vmem_limit_bytes=100 * 1024 * 1024),
    )(x, route, expert_W)
    out = out.reshape(TOK // 8, OR, 8, LANES).transpose(0, 2, 1, 3)
    return out.reshape(TOK, D_OUT)
```
